```python
import numpy as np

kernel_name = "dist_max_ax1_xy_m4096_n1024"

def setup_inputs():
    return {"x": np.random.randn(8192, 2048).astype(np.float32)}

def reference(x: np.ndarray) -> np.ndarray:
    return np.max(x, axis=1, keepdims=True)
```

```python
import jax
import jax.numpy as jnp
from jax import lax
from jax.experimental import pallas as pl
from jax.experimental.pallas import tpu as pltpu

M, N = 4096, 1024
G, PP = 32, 16
MESH = pl.DeviceIdType.MESH
NEG = float("-inf")


def tree_max(vs):
    vs = list(vs)
    while len(vs) > 1:
        vs = [jnp.maximum(vs[i], vs[i + 1]) if i + 1 < len(vs) else vs[i] for i in range(0, len(vs), 2)]
    return vs[0]


def make(nb=30, stages=None, depth=2, pattern=(0, 1), bounds=False, semchk=False, tail_pattern=None):
    if stages is None:
        seq = [(g, p) for p in range(PP) for g in range(nb, G)]
        last = [(G - 1, p) for p in range(12, 16)]
        seq = [t for t in seq if t not in last]
        stages = [seq[:-8], seq[-8:], last]
    assert sorted(t for s in stages for t in s) == [(g, p) for g in range(nb, G) for p in range(PP)]
    tail_pattern = tail_pattern or pattern
    ntail = (G - nb) * PP
    done_at = {}
    for k, s in enumerate(stages):
        for g, _ in s:
            done_at[g] = k
    sends = []
    for k in range(len(stages)):
        rows = sorted(g for g in done_at if done_at[g] == k)
        assert rows == list(range(rows[0], rows[-1] + 1)) if rows else True
        sends.append(rows)
    nmsg = 1 + sum(1 for r in sends if r)

    def body(x_hbm, o_ref, buf, tbuf, part, recv, wsem, tsem, ssem, rsem):
        def issue_wave(p):
            for g in range(nb):
                r = g * 128 + p * 8
                if not isinstance(r, int):
                    r = pl.multiple_of(r, 8)
                pltpu.make_async_copy(x_hbm.at[pl.ds(r, 8)], buf.at[p, pl.ds(g * 8, 8)], wsem.at[p]).start(
                    priority=pattern[g % len(pattern)])

        def issue_tail():
            i = 0
            for k, s in enumerate(stages):
                for g, p in s:
                    pltpu.make_async_copy(x_hbm.at[pl.ds(g * 128 + p * 8, 8)], tbuf.at[pl.ds(i * 8, 8)],
                                          tsem.at[k]).start(priority=tail_pattern[i % len(tail_pattern)])
                    i += 1

        for p in range(depth):
            issue_wave(p)

        peer = (lax.axis_index("x"), 1 - lax.axis_index("y"))
        bar = pltpu.get_barrier_semaphore()
        pl.semaphore_signal(bar, inc=1, device_id=peer, device_id_type=MESH)

        sub = lax.broadcasted_iota(jnp.int32, (8, 128), 0)
        lane = lax.broadcasted_iota(jnp.int32, (8, 128), 1)
        diag = (lane & 7) == sub
        cell = lane >> 3

        def piece_red(ref_rows):
            m = tree_max(ref_rows[:, c * 128:(c + 1) * 128] for c in range(N // 128))
            return jnp.max(m, axis=1, keepdims=True)

        def compute_wave(p, acc):
            acc = list(acc)
            for t in range(len(acc)):
                u = None
                for j in range(8):
                    g = t * 8 + j
                    if g >= nb:
                        break
                    red = piece_red(buf[p, pl.ds(g * 8, 8), :])
                    row = jnp.max(jnp.where(diag, red, NEG), axis=0, keepdims=True)
                    u = jnp.broadcast_to(row, (8, 128)) if u is None else jnp.where(sub == j, row, u)
                acc[t] = jnp.where(cell == p, u, acc[t])
            return tuple(acc)

        def wait_wave(p):
            pltpu.make_async_copy(buf.at[p], buf.at[p], wsem.at[p]).wait()

        def step(p, acc):
            wait_wave(p)

            @pl.when(p + depth < PP)
            def _():
                issue_wave(p + depth)

            @pl.when(p + depth == PP)
            def _():
                issue_tail()

            return compute_wave(p, acc)

        acc = tuple(jnp.full((8, 128), NEG, jnp.float32) for _ in range((nb + 7) // 8))
        acc = lax.fori_loop(0, PP, step, acc)
        for t in range(len(acc)):
            n = min(8, nb - t * 8)
            part[pl.ds(t * 8, n), :] = acc[t][:n]

        pl.semaphore_wait(bar, 1)

        def msg(i, r0, n):
            return pltpu.make_async_remote_copy(part.at[pl.ds(r0, n)], recv.at[pl.ds(r0, n)], ssem.at[i], rsem.at[i],
                                                device_id=peer, device_id_type=MESH)

        msgs = [(msg(0, 0, nb), 0, nb)]
        msgs[0][0].start()

        d = {g: jnp.full((8, 128), NEG, jnp.float32) for g in range(nb, G)}
        i = 0
        for k, s in enumerate(stages):
            rows = tbuf.at[pl.ds(i * 8, len(s) * 8)]
            pltpu.make_async_copy(rows, rows, tsem.at[k]).wait()
            for g, p in s:
                red = piece_red(tbuf[pl.ds(i * 8, 8), :])
                d[g] = jnp.where(lane == sub + 8 * p, red, d[g])
                i += 1
            if sends[k]:
                for g in sends[k]:
                    part[pl.ds(g, 1), :] = jnp.max(d[g], axis=0, keepdims=True)
                m = msg(len(msgs), sends[k][0], len(sends[k]))
                m.start()
                msgs.append((m, sends[k][0], len(sends[k])))

        for m, _, _ in msgs:
            m.wait_send()
        for m, r0, n in msgs:
            m.wait_recv()
            o_ref[pl.ds(r0, n), :] = jnp.maximum(part[pl.ds(r0, n), :], recv[pl.ds(r0, n), :])

    def fn(x):
        out = pl.pallas_call(
            body,
            out_shape=jax.ShapeDtypeStruct((G, 128), jnp.float32),
            in_specs=[pl.BlockSpec(memory_space=pl.ANY)],
            out_specs=pl.BlockSpec(memory_space=pltpu.VMEM),
            scratch_shapes=[
                pltpu.VMEM((PP, nb * 8, N), jnp.float32),
                pltpu.VMEM((ntail * 8, N), jnp.float32),
                pltpu.VMEM((G, 128), jnp.float32),
                pltpu.VMEM((G, 128), jnp.float32),
                pltpu.SemaphoreType.DMA((PP,)),
                pltpu.SemaphoreType.DMA((len(stages),)),
                pltpu.SemaphoreType.DMA((nmsg,)),
                pltpu.SemaphoreType.DMA((nmsg,)),
            ],
            compiler_params=pltpu.CompilerParams(
                collective_id=0, vmem_limit_bytes=32 * 1024 * 1024,
                disable_bounds_checks=not bounds, disable_semaphore_checks=not semchk),
        )(x)
        return out.reshape(M, 1)

    return fn


def pallas_dist_max_ax1_xy_m4096_n1024_kernel(x):
    return make(depth=4)(x)
```

```python
import jax
import jax.numpy as jnp
from jax import lax
from jax.experimental import pallas as pl
from jax.experimental.pallas import tpu as pltpu

ROWS, COLS = 4096, 1024
SUBLANES, LANES = 8, 128
TILES = COLS // LANES
SLABS = LANES // SUBLANES
GROUPS = ROWS // LANES
OWN = TILES - 1

BULK = 30
AHEAD = 3

FIRST_TAIL = BULK * SLABS
_EIGHT = (0, 4, 2, 6, 1, 5, 3, 7)
TAIL = (
    tuple(FIRST_TAIL + g * SLABS + p for p in range(8) for g in range(2))
    + tuple(FIRST_TAIL + 8 + p for p in _EIGHT)
    + tuple(FIRST_TAIL + SLABS + 8 + p for p in _EIGHT)
)
TAIL_STAGES = ((24,), (2, 2, 2, 2))
TAIL_ISSUED = (16, 19, 22)

NEG_INF = float("-inf")


def _tree_max(values):
    while len(values) > 1:
        pairs = [jnp.maximum(a, b) for a, b in zip(values[0::2], values[1::2])]
        values = pairs + values[2 * len(pairs):]
    return values[0]


def _kernel(x_hbm, out_ref, buf, bulk_max, bulk_peer, tail_max, tail_peer,
            wave_sems, tail_sems, send_sems, recv_sems):

    def fetch(slot, slab, prev_slab, sem, queue):
        for tile in (*range(OWN, TILES), *range(OWN)):
            row = (slab if tile < OWN else prev_slab) * SUBLANES
            if not isinstance(row, int):
                row = pl.multiple_of(row, SUBLANES)
            cols = pl.ds(tile * LANES, LANES)
            pltpu.make_async_copy(
                x_hbm.at[pl.ds(row, SUBLANES), cols], buf.at[slot, :, cols], sem
            ).start(priority=queue)

    def fetch_bulk(wave, group):
        slab = group * SLABS + wave
        prev = slab - 1 if group else jnp.where(wave == 0, FIRST_TAIL, slab) - 1
        fetch(wave * BULK + group, slab, prev, wave_sems.at[wave], group % 2)

    stage_sizes = [n for stages in TAIL_STAGES for n in stages]
    stage_of = [k for k, n in enumerate(stage_sizes) for _ in range(n)]

    def tail_prev(slab):
        return (GROUPS * SLABS if slab == FIRST_TAIL else slab) - 1

    def fetch_tail(i):
        fetch(FIRST_TAIL + i, TAIL[i], tail_prev(TAIL[i]),
              tail_sems.at[stage_of[i]], i % 2)

    def wait_slots(first, count, sem):
        slots = buf.at[pl.ds(first, count)]
        pltpu.make_async_copy(slots, slots, sem).wait()

    def tiles(slot, lo, hi):
        data = buf[slot, :, pl.ds(lo * LANES, (hi - lo) * LANES)]
        return [data[:, t * LANES:(t + 1) * LANES] for t in range(hi - lo)]

    sub = lax.broadcasted_iota(jnp.int32, (SUBLANES, LANES), 0)
    lane = lax.broadcasted_iota(jnp.int32, (SUBLANES, LANES), 1)
    diagonal = lane % SUBLANES == sub
    lane_slab = lane // SUBLANES

    def reduce_bulk(acc, p, next_slot, interleave):
        acc = list(acc)
        for group in range(BULK):
            interleave(group)
            slab = (tiles(p * BULK + group, 0, OWN)
                    + tiles(next_slot(group), OWN, TILES))
            column = jnp.max(_tree_max(slab), axis=1, keepdims=True)
            row = jnp.max(jnp.where(diagonal, column, NEG_INF), axis=0,
                          keepdims=True)
            place = (lane_slab == p) & (sub == group % SUBLANES)
            acc[group // SUBLANES] = jnp.where(place, row, acc[group // SUBLANES])
        return tuple(acc)

    @pl.loop(0, AHEAD)
    def _(wave):
        for group in range(BULK):
            fetch_bulk(wave, group)

    peer = (lax.axis_index("x"), 1 - lax.axis_index("y"))
    barrier = pltpu.get_barrier_semaphore()
    pl.semaphore_signal(barrier, inc=1, device_id=peer,
                        device_id_type=pl.DeviceIdType.MESH)

    def steady(p, acc):
        wait_slots((p + 1) * BULK, BULK, wave_sems.at[p + 1])
        return reduce_bulk(acc, p, lambda g: (p + 1) * BULK + g,
                           lambda g: fetch_bulk(p + AHEAD, g))

    wait_slots(0, BULK, wave_sems.at[0])
    acc = (jnp.full((SUBLANES, LANES), NEG_INF, jnp.float32),) * (GROUPS // SUBLANES)
    acc = lax.fori_loop(0, SLABS - AHEAD, steady, acc)

    issued = 0
    for p, upto in zip(range(SLABS - AHEAD, SLABS), TAIL_ISSUED):

        def interleave(group, lo=issued, n=upto - issued):
            for i in range(lo + n * group // BULK, lo + n * (group + 1) // BULK):
                fetch_tail(i)

        if p + 1 < SLABS:
            wait_slots((p + 1) * BULK, BULK, wave_sems.at[p + 1])
            acc = reduce_bulk(acc, p, lambda g: (p + 1) * BULK + g, interleave)
        else:
            acc = reduce_bulk(acc, p, lambda g: (g + 1) % BULK, interleave)
        issued = upto
    bulk_max[...] = jnp.concatenate(acc, axis=0)

    def send(index, src, dst):
        copy = pltpu.make_async_remote_copy(
            src, dst, send_sems.at[index], recv_sems.at[index],
            device_id=peer, device_id_type=pl.DeviceIdType.MESH)
        copy.start()
        return copy

    pl.semaphore_wait(barrier, 1)
    sends = [send(0, bulk_max, bulk_peer)]
    for i in range(issued, len(TAIL)):
        fetch_tail(i)

    folded = {}
    stage = first = 0
    for j, stages in enumerate(TAIL_STAGES):
        for count in stages:
            wait_slots(FIRST_TAIL + first, count, tail_sems.at[stage])
            for i in range(first, first + count):
                for slab, lo, hi in ((TAIL[i], 0, OWN),
                                     (tail_prev(TAIL[i]), OWN, TILES)):
                    count_so_far, partial = folded.get(slab, (0, []))
                    folded[slab] = (
                        count_so_far + hi - lo,
                        [_tree_max(tiles(FIRST_TAIL + i, lo, hi) + partial)])
            stage, first = stage + 1, first + count
        if j == 0:
            spread = [jnp.full((SUBLANES, LANES), NEG_INF, jnp.float32)] * 2
        for slab in sorted(s for s in folded if folded[s][0] == TILES):
            column = jnp.max(folded.pop(slab)[1][0], axis=1, keepdims=True)
            g, p = divmod(slab - FIRST_TAIL, SLABS)
            assert g >= j, "a tail group was sent before all its slabs landed"
            spread[g] = jnp.where(lane == sub + p * SUBLANES, column, spread[g])
        tail_max[j] = jnp.max(spread[j], axis=0, keepdims=True)
        sends.append(send(1 + j, tail_max.at[j], tail_peer.at[j]))
    assert not folded

    for copy in sends:
        copy.wait_send()
    sends[0].wait_recv()
    out_ref[...] = jnp.maximum(bulk_max[...], bulk_peer[...])
    for j, copy in enumerate(sends[1:]):
        mine = tail_max[j]
        copy.wait_recv()
        out_ref[pl.ds(BULK + j, 1), :] = jnp.maximum(mine, tail_peer[j])


def pallas_dist_max_ax1_xy_m4096_n1024_kernel(x: jax.Array):
    tail_groups = GROUPS - BULK
    out = pl.pallas_call(
        _kernel,
        out_shape=jax.ShapeDtypeStruct((GROUPS, LANES), jnp.float32),
        in_specs=[pl.BlockSpec(memory_space=pl.ANY)],
        out_specs=pl.BlockSpec(memory_space=pltpu.VMEM),
        scratch_shapes=[
            pltpu.VMEM((GROUPS * SLABS, SUBLANES, COLS), jnp.float32),
            pltpu.VMEM((GROUPS, LANES), jnp.float32),
            pltpu.VMEM((GROUPS, LANES), jnp.float32),
            pltpu.VMEM((tail_groups, 1, LANES), jnp.float32),
            pltpu.VMEM((tail_groups, 1, LANES), jnp.float32),
            pltpu.SemaphoreType.DMA((SLABS,)),
            pltpu.SemaphoreType.DMA((sum(map(len, TAIL_STAGES)),)),
            pltpu.SemaphoreType.DMA((1 + tail_groups,)),
            pltpu.SemaphoreType.DMA((1 + tail_groups,)),
        ],
        compiler_params=pltpu.CompilerParams(
            collective_id=0,
            vmem_limit_bytes=32 * 1024 * 1024,
            disable_semaphore_checks=True,
        ),
    )(x)
    return out.reshape(ROWS, 1)
```

```python
import jax
import jax.numpy as jnp
from jax import lax
from jax.experimental import pallas as pl
from jax.experimental.pallas import tpu as pltpu

ROWS, COLS = 4096, 1024
SUBLANES, LANES = 8, 128
TILES = COLS // LANES
SLABS = LANES // SUBLANES
GROUPS = ROWS // LANES
OWN = TILES - 1

COARSE = ((OWN, TILES - OWN), (0, OWN))
FINE = tuple((first + t, 1) for first, count in COARSE for t in range(count))

BULK = 30
AHEAD = 4

FIRST_TAIL = BULK * SLABS
_EIGHT = (0, 2, 1, 3, 4, 6, 5, 7)
TAIL = (
    tuple(FIRST_TAIL + g * SLABS + p for p in _EIGHT for g in range(2))
    + tuple(FIRST_TAIL + 8 + p for p in _EIGHT)
    + tuple(FIRST_TAIL + SLABS + 8 + p for p in _EIGHT)
)
TAIL_STAGES = ((24,), (2, 2, 2, 2))
TAIL_ISSUED = (8, 16, 19, 22)

NEG_INF = float("-inf")


def _tree_max(values):
    while len(values) > 1:
        pairs = [jnp.maximum(a, b) for a, b in zip(values[0::2], values[1::2])]
        values = pairs + values[2 * len(pairs):]
    return values[0]


def _tail_prev(slab):
    return (GROUPS * SLABS if slab == FIRST_TAIL else slab) - 1


def _kernel(x_hbm, out_ref, buf, bulk_max, bulk_peer, tail_max, tail_peer,
            wave_sems, tail_sems, send_sems, recv_sems):

    def fetch(slot, slab, prev_slab, sem, priority, parts):
        for tile, count in parts:
            row = (slab if tile < OWN else prev_slab) * SUBLANES
            if not isinstance(row, int):
                row = pl.multiple_of(row, SUBLANES)
            cols = pl.ds(tile * LANES, count * LANES)
            pltpu.make_async_copy(
                x_hbm.at[pl.ds(row, SUBLANES), cols], buf.at[slot, :, cols], sem
            ).start(priority=priority)

    def fetch_bulk(wave, group):
        slab = group * SLABS + wave
        fetch(wave * BULK + group, slab, slab - 1, wave_sems.at[wave],
              group % 2, COARSE)

    for group in range(BULK):
        slab = group * SLABS
        fetch(group, slab, (slab - 1) % FIRST_TAIL, wave_sems.at[0],
              group % 2, FINE)

    @pl.loop(1, AHEAD)
    def _(wave):
        for group in range(BULK):
            fetch_bulk(wave, group)

    peer = (lax.axis_index("x"), 1 - lax.axis_index("y"))
    barrier = pltpu.get_barrier_semaphore()
    pl.semaphore_signal(barrier, inc=1, device_id=peer,
                        device_id_type=pl.DeviceIdType.MESH)

    stage_sizes = [n for stages in TAIL_STAGES for n in stages]
    stage_of = [k for k, n in enumerate(stage_sizes) for _ in range(n)]

    def fetch_tail(i):
        fetch(FIRST_TAIL + i, TAIL[i], _tail_prev(TAIL[i]),
              tail_sems.at[stage_of[i]], i % 2, FINE)

    def wait_slots(first, count, sem):
        slots = buf.at[pl.ds(first, count)]
        pltpu.make_async_copy(slots, slots, sem).wait()

    def tiles(slot, lo, hi):
        data = buf[slot, :, pl.ds(lo * LANES, (hi - lo) * LANES)]
        return [data[:, t * LANES:(t + 1) * LANES] for t in range(hi - lo)]

    sub = lax.broadcasted_iota(jnp.int32, (SUBLANES, LANES), 0)
    lane = lax.broadcasted_iota(jnp.int32, (SUBLANES, LANES), 1)
    diagonal = (lane & (SUBLANES - 1)) == sub
    lane_slab = lane >> 3
    empty = jnp.full((SUBLANES, LANES), NEG_INF, jnp.float32)

    def reduce_bulk(acc, p, next_slot, interleave):
        acc = list(acc)
        for group in range(BULK):
            interleave(group)
            slab = (tiles(p * BULK + group, 0, OWN)
                    + tiles(next_slot(group), OWN, TILES))
            column = jnp.max(_tree_max(slab), axis=1, keepdims=True)
            row = jnp.max(jnp.where(diagonal, column, NEG_INF), axis=0,
                          keepdims=True)
            place = (lane_slab == p) & (sub == group % SUBLANES)
            acc[group // SUBLANES] = jnp.where(place, row, acc[group // SUBLANES])
        return tuple(acc)

    def steady(p, acc):
        wait_slots((p + 1) * BULK, BULK, wave_sems.at[p + 1])
        return reduce_bulk(acc, p, lambda g: (p + 1) * BULK + g,
                           lambda g: fetch_bulk(p + AHEAD, g))

    wait_slots(0, BULK, wave_sems.at[0])
    acc = lax.fori_loop(0, SLABS - AHEAD, steady, (empty,) * (GROUPS // SUBLANES))

    issued = 0
    for p, upto in zip(range(SLABS - AHEAD, SLABS), TAIL_ISSUED, strict=True):

        def interleave(group, lo=issued, n=upto - issued):
            for i in range(lo + n * group // BULK, lo + n * (group + 1) // BULK):
                fetch_tail(i)

        if p + 1 < SLABS:
            wait_slots((p + 1) * BULK, BULK, wave_sems.at[p + 1])
            acc = reduce_bulk(acc, p, lambda g: (p + 1) * BULK + g, interleave)
        else:
            acc = reduce_bulk(acc, p, lambda g: (g + 1) % BULK, interleave)
        issued = upto
    bulk_max[...] = jnp.concatenate(acc, axis=0)

    def send(index, src, dst):
        copy = pltpu.make_async_remote_copy(
            src, dst, send_sems.at[index], recv_sems.at[index],
            device_id=peer, device_id_type=pl.DeviceIdType.MESH)
        copy.start()
        return copy

    pl.semaphore_wait(barrier, 1)
    sends = [send(0, bulk_max, bulk_peer)]
    for i in range(issued, len(TAIL)):
        fetch_tail(i)

    started = {}
    spread = [empty] * len(TAIL_STAGES)
    stage = first = 0
    for j, stages in enumerate(TAIL_STAGES):
        finished = {}
        for count in stages:
            wait_slots(FIRST_TAIL + first, count, tail_sems.at[stage])
            for i in range(first, first + count):
                for slab, lo, hi in ((TAIL[i], 0, OWN),
                                     (_tail_prev(TAIL[i]), OWN, TILES)):
                    landed = tiles(FIRST_TAIL + i, lo, hi)
                    if slab in started:
                        finished[slab] = _tree_max(landed + started.pop(slab))
                    else:
                        started[slab] = [_tree_max(landed)]
            stage, first = stage + 1, first + count
        for slab in sorted(finished):
            g, p = divmod(slab - FIRST_TAIL, SLABS)
            assert g >= j, "a tail group was sent before all its slabs landed"
            column = jnp.max(finished[slab], axis=1, keepdims=True)
            spread[g] = jnp.where(lane == sub + p * SUBLANES, column, spread[g])
        tail_max[j] = jnp.max(spread[j], axis=0, keepdims=True)
        sends.append(send(1 + j, tail_max.at[j], tail_peer.at[j]))
    assert not started

    for copy in sends:
        copy.wait_send()
    sends[0].wait_recv()
    out_ref[...] = jnp.maximum(bulk_max[...], bulk_peer[...])
    for j, copy in enumerate(sends[1:]):
        mine = tail_max[j]
        copy.wait_recv()
        out_ref[pl.ds(BULK + j, 1), :] = jnp.maximum(mine, tail_peer[j])


def pallas_dist_max_ax1_xy_m4096_n1024_kernel(x: jax.Array):
    tail_groups = GROUPS - BULK
    out = pl.pallas_call(
        _kernel,
        out_shape=jax.ShapeDtypeStruct((GROUPS, LANES), jnp.float32),
        in_specs=[pl.BlockSpec(memory_space=pl.ANY)],
        out_specs=pl.BlockSpec(memory_space=pltpu.VMEM),
        scratch_shapes=[
            pltpu.VMEM((GROUPS * SLABS, SUBLANES, COLS), jnp.float32),
            pltpu.VMEM((GROUPS, LANES), jnp.float32),
            pltpu.VMEM((GROUPS, LANES), jnp.float32),
            pltpu.VMEM((tail_groups, 1, LANES), jnp.float32),
            pltpu.VMEM((tail_groups, 1, LANES), jnp.float32),
            pltpu.SemaphoreType.DMA((SLABS,)),
            pltpu.SemaphoreType.DMA((sum(map(len, TAIL_STAGES)),)),
            pltpu.SemaphoreType.DMA((1 + tail_groups,)),
            pltpu.SemaphoreType.DMA((1 + tail_groups,)),
        ],
        compiler_params=pltpu.CompilerParams(
            collective_id=0,
            vmem_limit_bytes=32 * 1024 * 1024,
            disable_semaphore_checks=True,
        ),
    )(x)
    return out.reshape(ROWS, 1)
```
